```python
import numpy as np

kernel_name = "dist_mlp2_tp_i_m512_h1024_out512"

def setup_inputs():
    x = np.random.randn(512, 512).astype(np.float32)
    W1 = np.random.randn(512, 4096).astype(np.float32)
    W2 = np.random.randn(4096, 512).astype(np.float32)
    return {"x": x, "W1": W1, "W2": W2}

def reference(x: np.ndarray, W1: np.ndarray, W2: np.ndarray) -> np.ndarray:
    h = x @ W1
    h = np.maximum(h, 0.0)
    return h @ W2
```

```python
import jax
import jax.numpy as jnp
from jax import lax
from jax.experimental import pallas as pl
from jax.experimental.pallas import tpu as pltpu

bf = jnp.bfloat16
f32 = jnp.float32
MESH = pl.DeviceIdType.MESH

import contextlib
def make(scopes=False):
    def sc(name):
        return jax.named_scope(name) if scopes else contextlib.nullcontext()

    def body(x_hbm, w1_hbm, w2_hbm, out_ref,
             xv, w1v, w2v, xb, hacc, hb, s1, r1, s2, r2, s3, r3,
             lsem, ssem, rsem):
        my = lax.axis_index("i")
        cx = my >> 1
        cy = (my ^ cx) & 1
        py = my ^ 1
        px = 3 - my
        ra = pl.multiple_of((1 - cy) * 128, 128)
        rb = pl.multiple_of(256 + (1 - cx) * 128, 128)
        rm1 = pl.multiple_of(cy * 128, 128)
        rm2 = pl.multiple_of(256 + cx * 128, 128)

        bar = pltpu.get_barrier_semaphore()
        for nbr in (py, px):
            pl.semaphore_signal(bar, inc=1, device_id=(nbr,), device_id_type=MESH)

        loads = []
        for q, r in enumerate((ra, rb, rm1, rm2)):
            loads.append(pltpu.make_async_copy(x_hbm.at[pl.ds(r, 128), :], xv.at[pl.ds(q * 128, 128), :], lsem.at[q]))
        for k in range(4):
            loads.append(pltpu.make_async_copy(w1_hbm.at[pl.ds(k * 128, 128), :], w1v.at[pl.ds(k * 128, 128), :], lsem.at[4 + k]))
        for c in range(4):
            loads.append(pltpu.make_async_copy(w2_hbm.at[:, pl.ds(c * 128, 128)], w2v.at[c], lsem.at[8 + c]))
        for l in loads:
            l.start()

        def rdma(stage, c, half, src, dst, dev):
            idx = (stage * 4 + c) * 2 + half
            return pltpu.make_async_remote_copy(
                src_ref=src.at[c, pl.ds(half * 128, 128), :], dst_ref=dst.at[c, pl.ds(half * 128, 128), :],
                send_sem=ssem.at[idx], recv_sem=rsem.at[idx], device_id=(dev,), device_id_type=MESH)

        d1 = [[rdma(0, c, 0, s1, r1, py), rdma(0, c, 1, s1, r1, px)] for c in range(4)]
        d2 = [[rdma(1, c, 0, s2, r2, px), rdma(1, c, 1, s2, r2, py)] for c in range(4)]
        d3 = [[rdma(2, c, 0, s3, r3, py), rdma(2, c, 1, s3, r3, px)] for c in range(4)]

        with sc("wait_x"):
            for q in range(4):
                loads[q].wait()
        with sc("cvt_x"):
            xb[...] = xv[...].astype(bf)
        for k in range(4):
            with sc(f"wait_w1_{k}"):
                loads[4 + k].wait()
            with sc(f"h_{k}"):
                p = jnp.dot(xb[:, k * 128:(k + 1) * 128], w1v[k * 128:(k + 1) * 128, :].astype(bf), preferred_element_type=f32)
                if k == 0:
                    hacc[...] = p
                elif k < 3:
                    hacc[...] += p
                else:
                    hb[...] = jnp.maximum(hacc[...] + p, 0.0).astype(bf)
        with sc("barrier"):
            pl.semaphore_wait(bar, 2)

        def stage2(c):
            with sc(f"w_r1_{c}"):
                d1[c][0].wait_recv(); d1[c][1].wait_recv()
            with sc(f"s2_{c}"):
                cs = pl.ds(c * 128, 128)
                t1 = out_ref[pl.ds(rm1, 128), cs] + r1[c, 0:128, :].astype(f32)
                t2 = out_ref[pl.ds(rm2, 128), cs] + r1[c, 128:256, :].astype(f32)
                s2[c, 0:128, :] = t1.astype(bf)
                s2[c, 128:256, :] = t2.astype(bf)
                d2[c][0].start(); d2[c][1].start()
                out_ref[pl.ds(rm1, 128), cs] = t1
                out_ref[pl.ds(rm2, 128), cs] = t2

        for c in range(4):
            with sc(f"wait_w2_{c}"):
                loads[8 + c].wait()
            with sc(f"s1_{c}"):
                w = w2v[c].astype(bf)
                s1[c] = jnp.dot(hb[0:256, :], w, preferred_element_type=f32).astype(bf)
                d1[c][0].start(); d1[c][1].start()
            with sc(f"om_{c}"):
                o = jnp.dot(hb[256:512, :], w2v[c].astype(bf), preferred_element_type=f32)
                cs = pl.ds(c * 128, 128)
                out_ref[pl.ds(rm1, 128), cs] = o[0:128]
                out_ref[pl.ds(rm2, 128), cs] = o[128:256]
        for c in range(4):
            stage2(c)
        for c in range(4):
            with sc(f"w_r2_{c}"):
                d2[c][0].wait_recv(); d2[c][1].wait_recv()
            with sc(f"s3_{c}"):
                cs = pl.ds(c * 128, 128)
                t1 = out_ref[pl.ds(rm1, 128), cs] + r2[c, 0:128, :].astype(f32)
                t2 = out_ref[pl.ds(rm2, 128), cs] + r2[c, 128:256, :].astype(f32)
                s3[c, 0:128, :] = t1.astype(bf)
                s3[c, 128:256, :] = t2.astype(bf)
                d3[c][0].start(); d3[c][1].start()
                out_ref[pl.ds(rm1, 128), cs] = t1
                out_ref[pl.ds(rm2, 128), cs] = t2
        for c in range(4):
            with sc(f"w_r3_{c}"):
                d3[c][0].wait_recv(); d3[c][1].wait_recv()
            with sc(f"fin_{c}"):
                cs = pl.ds(c * 128, 128)
                out_ref[pl.ds(ra, 128), cs] = r3[c, 0:128, :].astype(f32)
                out_ref[pl.ds(rb, 128), cs] = r3[c, 128:256, :].astype(f32)
        with sc("wait_sends"):
            for d in (d1, d2, d3):
                for c in range(4):
                    d[c][0].wait_send(); d[c][1].wait_send()

    def kernel(x, W1, W2):
        comm = pltpu.VMEM((4, 256, 128), bf)
        return pl.pallas_call(
            body,
            out_shape=jax.ShapeDtypeStruct((512, 512), f32),
            in_specs=[pl.BlockSpec(memory_space=pl.ANY)] * 3,
            out_specs=pl.BlockSpec(memory_space=pltpu.VMEM),
            scratch_shapes=[
                pltpu.VMEM((512, 512), f32), pltpu.VMEM((512, 1024), f32), pltpu.VMEM((4, 1024, 128), f32),
                pltpu.VMEM((512, 512), bf), pltpu.VMEM((512, 1024), f32), pltpu.VMEM((512, 1024), bf),
                comm, comm, comm, comm, comm, comm,
                pltpu.SemaphoreType.DMA((12,)), pltpu.SemaphoreType.DMA((24,)), pltpu.SemaphoreType.DMA((24,)),
            ],
            compiler_params=pltpu.CompilerParams(collective_id=0, disable_semaphore_checks=True),
        )(x, W1, W2)
    return kernel


def pallas_dist_mlp2_tp_i_m512_h1024_out512_kernel(x, W1, W2):
    return make(False)(x, W1, W2)
```

```python
import jax
import jax.numpy as jnp
from jax import lax
from jax.experimental import pallas as pl
from jax.experimental.pallas import tpu as pltpu

bf = jnp.bfloat16
f32 = jnp.float32
MESH = pl.DeviceIdType.MESH
G = 64
NBR = ((1, 3), (0, 2), (3, 1), (2, 0))


def _path(a, b, c, d):
    return {(a, b): None, (b, c): a, (c, d): b, (d, c): None, (c, b): d, (b, a): c}


ROUTES = {'A0': _path(1, 0, 3, 2), 'A1': _path(0, 1, 2, 3), 'B0': _path(3, 0, 1, 2), 'B1': _path(0, 3, 2, 1)}
ROUTES['P3'] = {**{k: v for k, v in ROUTES['A1'].items() if k != (2, 3)}, (0, 3): 1}
ROUTES['P1'] = {**{k: v for k, v in ROUTES['B1'].items() if k != (2, 1)}, (0, 1): 3}
GETS_TOTAL = (('P3', 3), ('P1', 1))


def _zip_steps(lists, span):
    nxt = {i: 0 for i in lists}
    while True:
        live = [i for i in lists if nxt[i] < len(lists[i])]
        if not live:
            return
        rows = span(lists[live[0]][nxt[live[0]]][1])
        step = {i: tuple(lists[i][nxt[i]]) for i in live if span(lists[i][nxt[i]][1]) == rows}
        for i in step:
            nxt[i] += 1
        yield step


def build(T):
    tiles, lo, src, w1o, w2o, xord, role = T['tiles'], T['lo'], T['src'], T['w1o'], T['w2o'], T['xord'], T['role']
    xm, pre, post, tail = T['xm'], T['pre'], T['post'], T['tail']
    roles = [ro for ro in (1, 0, 2) if ro in role]
    members = {ro: [i for i in range(4) if role[i] == ro] for ro in roles}
    pos = [[lo[i].index(g) for g in range(8)] for i in range(4)]
    col = [[w2o[i].index(c) for c in range(4)] for i in range(4)]
    kloc = [[w1o[i].index(k) for k in range(4)] for i in range(4)]
    units = []
    for i in range(4):
        us = []
        for p in range(8):
            for g in xord[i]:
                k = 0
                while k < 4:
                    k0 = k
                    while k < 4 and src[i][g * 4 + k] == p:
                        k += 1
                    if k > k0:
                        us.append((p, g, k0, k))
                    else:
                        k += 1
        units.append(us)
    nt = len(tiles)
    dummy = 2 * nt
    lcell = lambda i, z: pos[i][tiles[z][0]] * 4 + col[i][tiles[z][1]]
    ridx = lambda s, d, z: NBR[d].index(s) * nt + z
    pred = lambda s, d, z: ROUTES[tiles[z][4]][(s, d)]
    span = lambda z: tuple(tiles[z][2:4])
    steps = lambda lists: _zip_steps(lists, span)
    n_xsend = max(len(m) for m in xm)
    n_sb, n_send = 0, 0
    for ro in roles:
        cs, nb = members[ro], len(T['blocks'][ro])
        count = lambda lists: sum(1 for _ in steps(lists))
        n_sb = max(n_sb, 32
                   + sum(count({i: [m for m in post[i][b] if pred(i, *m) is not None] for i in cs}) for b in range(nb))
                   + max(sum(op[0] == 'm' and pred(i, *op[1:]) is not None for op in tail[i][0]) for i in cs))
        n_send = max(n_send, n_xsend + 2 * sum(T['split'][ro])
                     + sum(count({i: pre[i][b] for i in cs}) + count({i: post[i][b] for i in cs}) for b in range(nb))
                     + max(sum(op[0] == 'm' for op in tail[i][0]) for i in cs))

    def body(x_hbm, w1_hbm, w2_hbm, out_ref,
             xf, w1v, w2v, xb, hacc, hb, P, SB, R, lsem, xsem, rsem, ssem):
        my = lax.axis_index("i")
        bar = pltpu.get_barrier_semaphore()

        def among(chips):
            mask = sum(1 << i for i in chips)
            return (lax.shift_right_logical(jnp.int32(mask), my) & 1) == 1

        def rcopy(s_ref, d_ref, s_sem, r_sem, dev):
            return pltpu.make_async_remote_copy(src_ref=s_ref, dst_ref=d_ref, send_sem=s_sem, recv_sem=r_sem,
                                                device_id=(dev,), device_id_type=MESH)

        def x_load(i, n):
            _, g, k0, k1 = units[i][n]
            cols = pl.ds(k0 * 128, (k1 - k0) * 128)
            return pltpu.make_async_copy(x_hbm.at[pl.ds(g * G, G), cols], xf.at[g, :, cols], lsem.at[8 + n])

        def x_tile(k, p):
            return xb.at[k, pl.ds(p * G, G), :]

        def wait_recv(r, r0, nr):
            ref = R.at[r, pl.ds(r0, nr), :]
            rcopy(ref, ref, ssem.at[0], rsem.at[r], 0).wait_recv()

        def wait_send(n, idx):
            ref = SB.at[idx[0], pl.ds(idx[1], idx[2]), :] if len(idx) == 3 else x_tile(*idx)
            rcopy(ref, ref, ssem.at[n], rsem.at[0], 0).wait_send()

        def relay_sum(n, a, r, r0, nr):
            SB[n, r0:r0 + nr, :] = (P[a, r0:r0 + nr, :] + R[r, r0:r0 + nr, :].astype(f32)).astype(bf)

        def start_loads(i):
            mixed = T['il'][i] * 256

            def w1_load(j, r0, n):
                pltpu.make_async_copy(w1_hbm.at[pl.ds(w1o[i][j] * 128 + r0, n), :], w1v.at[j, pl.ds(r0, n), :],
                                      lsem.at[j]).start()

            def w2_load(j, r0, n):
                pltpu.make_async_copy(w2_hbm.at[pl.ds(r0, n), pl.ds(w2o[i][j] * 128, 128)], w2v.at[j, pl.ds(r0, n), :],
                                      lsem.at[4 + j]).start()

            for p in range(8):
                for n, u in enumerate(units[i]):
                    if u[0] == p:
                        x_load(i, n).start()
                        if n == 0:
                            for nbr in NBR[i]:
                                pl.semaphore_signal(bar, inc=1, device_id=(nbr,), device_id_type=MESH)
                if p == 3:
                    n = 4 if mixed else 1
                    for q in range(n):
                        if mixed:
                            w2_load(0, q * mixed // 4, mixed // 4)
                        w1_load(3, q * 128 // n, 128 // n)
                elif p < 4:
                    w1_load(p, 0, 128)
                else:
                    r0 = mixed if p == 4 else 0
                    w2_load(p - 4, r0, 1024 - r0)

        for i in (2, 1, 3, 0):
            pl.when(my == i)(lambda i=i: start_loads(i))
        R[dummy] = jnp.zeros((G, 128), bf)

        def program(ro):
            cs = members[ro]
            blocks, heads, borrow = T['blocks'][ro], T['heads'][ro], T['borrow'][ro]
            W, split, slotp = T['W'][ro], T['split'][ro], T['slotp'][ro]
            nb = len(blocks)
            sent = {i: {} for i in cs}
            waited = {i: set() for i in cs}
            xstate = {i: dict(u=0, q=0, have=set(), synced=False) for i in cs}
            hcount = [0] * 8
            cnt = dict(send=n_xsend, sb=32)
            got = set()
            flying = {}

            def sel(f):
                vals = {i: f(i) for i in cs}
                if len(set(vals.values())) == 1:
                    return vals[cs[0]]
                packed = sum(v << (8 * i) for i, v in vals.items())
                return lax.shift_right_logical(jnp.int32(packed), my * 8) & 255

            def guarded(chips, fn):
                if len(chips) == len(cs):
                    fn()
                elif chips:
                    pl.when(among(chips))(fn)

            def run(ops):
                for op in ops:
                    op()

            def x_sends(i):
                st, ops = xstate[i], []
                while st['q'] < len(xm[i]) and tuple(xm[i][st['q']][1:]) in st['have']:
                    if not st['synced']:
                        ops.append(lambda: pl.semaphore_wait(bar, 2))
                        st['synced'] = True
                    q = st['q']
                    st['q'] += 1
                    d, g, k = xm[i][q]
                    here, there = (kloc[i][k], pos[i][g]), (kloc[d][k], pos[d][g])
                    sent[i]['x', q] = (q, here)
                    ops.append(lambda q=q, d=d, here=here, there=there: rcopy(
                        x_tile(*here), x_tile(*there), ssem.at[q], xsem.at[there[1] * 4 + there[0]], d).start())
                return ops

            def x_convert(i, n):
                _, g, k0, k1 = units[i][n]
                x_load(i, n).wait()
                p = pos[i][g]
                for k in range(k0, k1):
                    xb[kloc[i][k], p * G:(p + 1) * G, :] = xf[g, :, k * 128:(k + 1) * 128].astype(bf)

            def x_step(i, b):
                st, ops = xstate[i], []
                while st['u'] < len(units[i]) and slotp[units[i][st['u']][0]] <= b:
                    _, g, k0, k1 = units[i][st['u']]
                    ops.append(lambda n=st['u']: x_convert(i, n))
                    st['u'] += 1
                    st['have'].update((g, k) for k in range(k0, k1))
                    ops += x_sends(i)
                if not st['synced']:
                    ops.append(lambda: pl.semaphore_wait(bar, 2))
                    st['synced'] = True
                return ops

            def h_raw(ps, ks):
                lhs = jnp.concatenate(
                    [jnp.concatenate([xb[k, p * G:(p + 1) * G, :] for p in ps], axis=0) for k in ks], axis=1)
                rhs = jnp.concatenate([w1v[k].astype(bf) for k in ks], axis=0)
                return jnp.dot(lhs, rhs, preferred_element_type=f32)

            def h_dot(ps, ks):
                val = h_raw(ps, ks[:1])
                for n in range(1, len(ks)):
                    val = val + h_raw(ps, ks[n:n + 1])
                parts = [val[n * G:(n + 1) * G, :] for n in range(len(ps))]
                return [v + hacc[p * G:(p + 1) * G, :] if hcount[p] else v for p, v in zip(ps, parts)]

            def h_store(ps, ks, vals):
                for p, v in zip(ps, vals):
                    hcount[p] += len(ks)
                    if hcount[p] == 4:
                        v = jnp.maximum(v, 0.0).astype(bf)
                        for j in range(8):
                            hb[j, p * G:(p + 1) * G, :] = v[:, j * 128:(j + 1) * 128]
                    else:
                        hacc[p * G:(p + 1) * G, :] = v

            def o_dot(ps, j, r0=0, nr=G):
                lhs = jnp.concatenate(
                    [jnp.concatenate([hb[t, p * G + r0:p * G + r0 + nr, :] for p in ps], axis=0) for t in range(8)],
                    axis=1)
                return jnp.dot(lhs, w2v[j].astype(bf), preferred_element_type=f32)

            def o_store(ps, j, val, r0=0, nr=G):
                for n, p in enumerate(ps):
                    v = val[n * nr:(n + 1) * nr, :]
                    P[p * 4 + j, r0:r0 + nr, :] = v
                    SB[p * 4 + j, r0:r0 + nr, :] = v.astype(bf)

            def launch(ts):
                groups = {}
                for t in ts:
                    if t not in flying:
                        groups.setdefault((t[0], t[2]), []).append(t)
                for (o, k), group in groups.items():
                    ps = [t[1] for t in group]
                    val = o_dot(ps, k) if o == 'O' else h_raw(ps, (k,))
                    for n, t in enumerate(group):
                        flying[t] = val[n * G:(n + 1) * G, :]

            def land(t):
                o, p, k = t
                v = flying[t]
                if o == 'O':
                    o_store([p], k, v)
                else:
                    if hcount[p]:
                        v = jnp.concatenate(
                            [v[:, c:c + 512] + hacc[p * G:(p + 1) * G, c:c + 512] for c in (0, 512)], axis=1)
                    h_store([p], (k,), [v])

            def ahead(b):
                ts = [blocks[b][q] for q in heads[b]] if b < nb else []
                if b + 1 < nb and borrow[b + 1] and not split[b]:
                    ts.append(blocks[b + 1][heads[b + 1][0]])
                return ts

            def need(ts):
                items = {(o, k) for o, _, k in ts} - got | {('x', p, k) for o, p, k in ts if o == 'H'}
                got.update(items)
                for item in T['order'][ro]:
                    if item not in items:
                        continue
                    if item[0] == 'x':
                        _, p, k = item
                        guarded([i for i in cs if src[i][lo[i][p] * 4 + w1o[i][k]] >= 10], lambda: rcopy(
                            x_tile(k, p), x_tile(k, p), ssem.at[0], xsem.at[p * 4 + k], 0).wait_recv())
                    else:
                        o, k = item
                        buf, sem = (w2v.at[k], lsem.at[4 + k]) if o == 'O' else (w1v.at[k], lsem.at[k])
                        pltpu.make_async_copy(buf, buf, sem).wait()

            def send(ms, sidx, part=None):
                ref = min(ms)
                r0, nr = span(ms[ref][1])
                if part is not None and part[0] > 0:
                    n = sent[ref][ms[ref]][0]
                else:
                    n = cnt['send']
                    cnt['send'] += 1
                pick = lambda f: sel(lambda i: f(i if i in ms else ref))
                s, r, d = pick(sidx), pick(lambda i: ridx(i, *ms[i])), pick(lambda i: ms[i][0])
                for i in ms:
                    sent[i][ms[i]] = (n, (sidx(i), r0, nr))
                rows = pl.ds(*(part or (r0, nr)))
                guarded(list(ms), lambda: rcopy(SB.at[s, rows, :], R.at[r, rows, :], ssem.at[n], rsem.at[r], d).start())

            def early(b):
                out = {i: [] for i in cs}
                if b > 0 and split[b - 1]:
                    cells = [p * 4 + j for _, p, j in blocks[b - 1]]
                    for i in cs:
                        seen = set()
                        for m in pre[i][b]:
                            if m[0] not in seen and lcell(i, m[1]) in cells and span(m[1])[1] == G:
                                out[i].append(tuple(m))
                            seen.add(m[0])
                return out

            def relays(b):
                for ms in steps({i: [m for m in post[i][b] if pred(i, *m) is not None] for i in cs}):
                    yield ms, lambda i, ms=ms: ridx(pred(i, *ms[i]), i, ms[i][1]) if i in ms else dummy

            def relay_waits(b):
                for ms, rs in relays(b):
                    r = sel(rs)
                    guarded(list(ms), lambda: wait_recv(r, *span(ms[min(ms)][1])))
                    for i in ms:
                        waited[i].add(rs(i))

            def slot(b):
                first = early(b)
                for ms in steps(first):
                    send(ms, lambda i: lcell(i, ms[i][1]), (G // 2, G // 2))
                for ms in steps({i: [m for m in pre[i][b] if tuple(m) not in first[i]] for i in cs}):
                    send(ms, lambda i: lcell(i, ms[i][1]))
                if W[b]:
                    relay_waits(b)
                where = {}
                for ms, rs in relays(b):
                    ref = min(ms)
                    a = sel(lambda i: lcell(i, ms[i][1]) if i in ms else lcell(ref, ms[ref][1]))
                    relay_sum(cnt['sb'], a, sel(rs), *span(ms[ref][1]))
                    for i in ms:
                        where[i, ms[i]] = cnt['sb']
                    cnt['sb'] += 1
                for ms in steps({i: post[i][b] for i in cs}):
                    send(ms, lambda i: where.get((i, ms[i]), lcell(i, ms[i][1])))

            for b in range(nb):
                slot(b)
                for i in cs:
                    ops = x_step(i, b)
                    if ops:
                        guarded([i], lambda: run(ops))
                if W[b]:
                    e = b + 1
                    while e < nb and not W[e]:
                        relay_waits(e)
                        e += 1
                    todo = [t for z in range(b, e) for t in blocks[z]]
                    need(todo)
                    for i in cs:
                        xstate[i]['have'].update((lo[i][p], w1o[i][k]) for o, p, k in todo if o == 'H')
                        ops = x_sends(i)
                        if ops:
                            guarded([i], lambda: run(ops))
                tasks = [t for q, t in enumerate(blocks[b]) if q not in heads[b]]
                if not tasks:
                    launch(ahead(b + 1))
                for q in heads[b]:
                    land(blocks[b][q])
                if split[b]:
                    ps, j = [t[1] for t in tasks], tasks[0][2]
                    parts = ((0, 32), (32, 32)) if split[b] == 1 else ((0, 16), (16, 16), (32, 32))
                    vals = [o_dot(ps, j, *part) for part in parts]
                    for n, part in enumerate(parts[:-1]):
                        if borrow[b + 1] and n == len(parts) - 2:
                            launch([blocks[b + 1][heads[b + 1][0]]])
                        o_store(ps, j, vals[n], *part)
                        for ms in steps(early(b + 1)):
                            send(ms, lambda i: lcell(i, ms[i][1]), part)
                    launch(ahead(b + 1))
                    o_store(ps, j, vals[-1], *parts[-1])
                    continue
                ks, hg, og = {}, {}, {}
                for o, p, k in tasks:
                    if o == 'H':
                        ks[p] = ks.get(p, ()) + (k,)
                    else:
                        og.setdefault(k, []).append(p)
                for p, r in ks.items():
                    hg.setdefault(r, []).append(p)
                jobs = [(h_dot, h_store, ps, r) for r, ps in hg.items()]
                jobs += [(o_dot, o_store, ps, j) for j, ps in og.items()]
                for n, (dot, store, ps, r) in enumerate(jobs):
                    val = dot(ps, r)
                    if n == len(jobs) - 1:
                        launch(ahead(b + 1))
                    store(ps, r, val)

            def finish(i):
                assert xstate[i]['q'] == len(xm[i]) and xstate[i]['u'] == len(units[i])
                ops, late = tail[i]
                late = [tuple(m) for m in late]
                out, seen = dict(sent[i]), set(waited[i])
                ns, nr = cnt['send'], cnt['sb']

                def arrive(r, z):
                    if r not in seen:
                        seen.add(r)
                        wait_recv(r, *span(z))

                for op in ops:
                    if op[0] == 'm':
                        d, z = op[1:]
                        s = lcell(i, z)
                        r0, rn = span(z)
                        if pred(i, d, z) is not None:
                            r = ridx(pred(i, d, z), i, z)
                            arrive(r, z)
                            relay_sum(nr, s, r, r0, rn)
                            s = nr
                            nr += 1
                        r = ridx(i, d, z)
                        rows = pl.ds(r0, rn)
                        rcopy(SB.at[s, rows, :], R.at[r, rows, :], ssem.at[ns], rsem.at[r], d).start()
                        out[d, z] = (ns, (s, r0, rn))
                        ns += 1
                    elif op[0] == 'f':
                        z = op[1]
                        g, c, r0, rn, route = tiles[z]
                        rs = [ridx(s, i, z) for (s, d) in ROUTES[route] if d == i]
                        for r in rs:
                            arrive(r, z)
                        v = R[rs[0], r0:r0 + rn, :].astype(f32)
                        if len(rs) > 1:
                            v = v + R[rs[1], r0:r0 + rn, :].astype(f32)
                        if (route, i) not in GETS_TOTAL:
                            v = v + P[lcell(i, z), r0:r0 + rn, :]
                        out_ref[g * G + r0:g * G + r0 + rn, c * 128:(c + 1) * 128] = v
                    else:
                        for m, n in out.items():
                            if (m in late) == (op[1] == 'late'):
                                wait_send(*n)

            for i in reversed(cs):
                guarded([i], lambda i=i: finish(i))

        for ro in roles:
            pl.when(among(members[ro]))(lambda ro=ro: program(ro))

    def kernel(x, W1, W2):
        return pl.pallas_call(
            body,
            out_shape=jax.ShapeDtypeStruct((512, 512), f32),
            in_specs=[pl.BlockSpec(memory_space=pl.ANY)] * 3,
            out_specs=pl.BlockSpec(memory_space=pltpu.VMEM),
            scratch_shapes=[
                pltpu.VMEM((8, G, 512), f32),
                pltpu.VMEM((4, 128, 1024), f32),
                pltpu.VMEM((4, 1024, 128), f32),
                pltpu.VMEM((4, 512, 128), bf),
                pltpu.VMEM((512, 1024), f32),
                pltpu.VMEM((8, 512, 128), bf),
                pltpu.VMEM((32, G, 128), f32),
                pltpu.VMEM((n_sb, G, 128), bf),
                pltpu.VMEM((dummy + 1, G, 128), bf),
                pltpu.SemaphoreType.DMA((8 + max(len(u) for u in units),)),
                pltpu.SemaphoreType.DMA((32,)),
                pltpu.SemaphoreType.DMA((dummy + 1,)),
                pltpu.SemaphoreType.DMA((n_send,)),
            ],
            compiler_params=pltpu.CompilerParams(collective_id=0, disable_semaphore_checks=True),
        )(x, W1, W2)
    return kernel


PLAN = {'W': ((1, 1, 1, 1, 1, 1, 0, 0, 1, 0, 0, 1, 0, 0, 1, 1, 1, 0, 1, 0),
       (1, 1, 1, 1, 1, 1, 1, 1, 0, 0, 0, 1, 0, 0, 1, 0, 1, 1, 1, 1, 1, 1, 1, 1, 1, 1, 1)),
 'blocks': (((('H', 1, 0), ('H', 2, 0), ('H', 4, 0), ('H', 6, 0), ('H', 7, 0)),
             (('H', 3, 0), ('H', 1, 1), ('H', 2, 1), ('H', 3, 1), ('H', 4, 1), ('H', 6, 1), ('H', 7, 1)),
             (('H', 1, 2), ('H', 2, 2), ('H', 3, 2), ('H', 4, 2), ('H', 6, 2), ('H', 7, 2)),
             (('H', 1, 3), ('H', 3, 3), ('H', 6, 3)), (('H', 2, 3), ('H', 4, 3), ('H', 7, 3)),
             (('O', 2, 0), ('O', 6, 0)), (('O', 1, 0), ('O', 3, 0)),
             (('H', 0, 3), ('H', 5, 3), ('O', 4, 0), ('O', 7, 0)), (('O', 1, 1), ('O', 3, 1)),
             (('H', 0, 2), ('O', 4, 1), ('O', 7, 1)), (('H', 0, 1), ('H', 5, 1), ('O', 2, 1), ('O', 6, 1)),
             (('H', 0, 0), ('O', 2, 2), ('O', 6, 2)), (('H', 5, 0), ('H', 5, 2)), (('O', 0, 1), ('O', 5, 1)),
             (('O', 4, 2), ('O', 7, 2)), (('O', 0, 0), ('O', 5, 0)), (('O', 0, 2), ('O', 5, 2)),
             (('O', 1, 2), ('O', 3, 2), ('O', 3, 3)), (('O', 2, 3), ('O', 4, 3), ('O', 7, 3)),
             (('O', 0, 3), ('O', 1, 3), ('O', 5, 3), ('O', 6, 3))),
            ((('H', 0, 0), ('H', 4, 0), ('H', 5, 0), ('H', 6, 0)), (('H', 0, 1), ('H', 4, 1), ('H', 6, 1)),
             (('H', 7, 0), ('H', 1, 1), ('H', 5, 1)), (('H', 0, 2), ('H', 1, 2), ('H', 5, 2)),
             (('H', 1, 0), ('H', 4, 2), ('H', 6, 2)), (('H', 0, 3), ('H', 1, 3)), (('H', 4, 3), ('H', 6, 3)),
             (('O', 4, 0),), (('O', 0, 0), ('O', 6, 0)), (('H', 5, 3),), (('H', 7, 2), ('O', 1, 0), ('O', 5, 0)),
             (('O', 4, 1), ('O', 5, 1)), (('O', 1, 1), ('O', 6, 1)),
             (('H', 2, 1), ('H', 7, 1), ('H', 7, 3), ('O', 0, 1)), (('O', 0, 2), ('O', 4, 2)),
             (('O', 1, 2), ('O', 6, 2)), (('H', 2, 0), ('H', 2, 2), ('H', 2, 3), ('O', 7, 0)),
             (('O', 2, 0), ('O', 4, 3)), (('O', 7, 1), ('O', 6, 3)), (('O', 2, 1), ('O', 0, 3), ('O', 1, 3)),
             (('H', 3, 1),), (('H', 3, 0), ('H', 3, 2), ('H', 3, 3), ('O', 5, 2)), (('O', 3, 1),),
             (('O', 3, 0), ('O', 2, 2)), (('O', 2, 3), ('O', 3, 3), ('O', 7, 3)), (('O', 3, 2), ('O', 5, 3)),
             (('O', 7, 2),))),
 'borrow': ((0, 0, 0, 0, 0, 0, 1, 0, 0, 0, 0, 0, 0, 0, 0, 0, 0, 0, 0, 0),
            (0, 0, 0, 0, 0, 0, 0, 0, 0, 0, 1, 0, 1, 0, 0, 1, 0, 0, 0, 0, 0, 0, 0, 0, 0, 0, 0)),
 'heads': (((), (), (), (), (), (), (0, 1), (2, 3), (), (1, 2), (2, 3), (), (0, 1), (0,), (), (), (), (0, 1), (0,),
            (0,)),
           ((), (), (), (), (), (), (), (), (0, 1), (0,), (1, 0), (), (0, 1), (0, 1), (), (0, 1), (3,), (), (), (), (),
            (3,), (), (0,), (0,), (), ())),
 'il': (0, 1, 0, 1),
 'lo': ((3, 0, 1, 4, 2, 7, 5, 6), (4, 1, 3, 6, 7, 0, 2, 5), (6, 5, 4, 1, 7, 2, 0, 3), (0, 5, 7, 2, 3, 4, 6, 1)),
 'order': ((('x', 0, 0), ('x', 1, 0), ('x', 1, 1), ('x', 1, 2), ('x', 2, 0), ('x', 3, 0), ('x', 3, 1), ('x', 3, 2),
            ('x', 4, 0), ('x', 5, 0), ('x', 6, 0), ('x', 7, 0), ('H', 0), ('x', 4, 1), ('x', 7, 1), ('H', 1),
            ('x', 2, 1), ('x', 6, 1), ('x', 2, 2), ('x', 6, 2), ('H', 2), ('x', 4, 2), ('x', 7, 2), ('x', 2, 3),
            ('x', 6, 3), ('H', 3), ('x', 1, 3), ('x', 3, 3), ('x', 4, 3), ('x', 7, 3), ('O', 0), ('x', 0, 3),
            ('x', 5, 3), ('x', 0, 2), ('x', 5, 2), ('x', 0, 1), ('x', 5, 1), ('O', 1), ('O', 2), ('O', 3)),
           (('x', 0, 0), ('x', 1, 1), ('x', 3, 0), ('x', 3, 2), ('x', 3, 3), ('x', 4, 0), ('x', 4, 2), ('x', 5, 0),
            ('x', 5, 2), ('x', 6, 0), ('x', 6, 1), ('H', 0), ('x', 4, 1), ('H', 1), ('x', 0, 1), ('x', 7, 0),
            ('x', 5, 1), ('H', 2), ('x', 1, 2), ('x', 0, 2), ('x', 1, 0), ('x', 6, 2), ('x', 0, 3), ('H', 3),
            ('x', 1, 3), ('x', 4, 3), ('x', 6, 3), ('O', 0), ('x', 7, 2), ('x', 5, 3), ('x', 7, 3), ('x', 2, 1),
            ('x', 2, 0), ('O', 1), ('x', 7, 1), ('x', 2, 3), ('x', 3, 1), ('x', 2, 2), ('O', 2), ('O', 3))),
 'post': (((), (), (), (), (), (), (), (), (), (), (), (), (), (), (), (), ((3, 30), (1, 14)), (), ((3, 6), (1, 22)),
           ((3, 7),)),
          ((), (), (), (), (), (), (), (), (), (), (), (), (), (), ((2, 18),), (), ((0, 3),), ((0, 23),),
           ((0, 32), (0, 15)), ((0, 22),), ((0, 14),), ((0, 18),), ((0, 1), (2, 14)), ((2, 26), (0, 26)),
           ((2, 22), (0, 13)), ((2, 20), (0, 27)), ((2, 25), (0, 25))),
          ((), (), (), (), (), (), (), (), ((1, 32), (3, 33)), (), (), ((3, 2), (1, 18)), (), (), ((3, 10), (1, 26)),
           ((3, 29), (1, 13)), ((3, 11), (1, 27)), ((3, 9), (1, 25)), ((3, 5), (1, 21)), ((3, 28), (1, 12))),
          ((), (), (), (), (), (), (), (), (), (), (), (), (), (), ((2, 2),), (), ((0, 19),), ((0, 7),),
           ((0, 33), (0, 31)), ((0, 6),), ((0, 30),), ((0, 2),), ((0, 17), (2, 30)), ((2, 10), (0, 10)),
           ((2, 6), (0, 29)), ((2, 4), (0, 11)), ((2, 9), (0, 9)))),
 'pre': (((), (), (), (), (), (), (), ((3, 2), (1, 18)), ((3, 10), (1, 26)), ((3, 16), (1, 0)), ((3, 8), (1, 24)),
          ((3, 4), (1, 20)), ((3, 5), (1, 21)), (), ((3, 28), (1, 12)), ((3, 9), (1, 25)), (), ((3, 29), (1, 13)), (),
          ((1, 27),)),
         ((), (), (), (), (), (), (), (), ((0, 31), (2, 33)), ((0, 19), (2, 11)), (), ((0, 7),), ((2, 2), (0, 30)),
          ((2, 10), (0, 6)), (), ((0, 17), (2, 29)), ((2, 9), (2, 5)), (), ((2, 28),), ((2, 8),), ((2, 16), (2, 4)), (),
          (), (), (), (), ()),
         ((), (), (), (), (), (), ((3, 19), (1, 3)), ((3, 7), (1, 23)), ((3, 31), (1, 15)), ((3, 6), (1, 22)),
          ((3, 30), (1, 14)), (), ((3, 17), (1, 1)), (), (), (), (), (), (), ()),
         ((), (), (), (), (), (), (), (), ((0, 15), (2, 32)), ((0, 3), (2, 27)), (), ((0, 23),), ((2, 18), (0, 14)),
          ((2, 26), (0, 22)), (), ((0, 1), (2, 13)), ((2, 25), (2, 21)), (), ((2, 12),), ((2, 24),), ((2, 0), (2, 20)),
          (), (), (), (), (), ())),
 'role': (0, 1, 0, 1),
 'slotp': ((0, 1, 2, 3, 5, 8, 11, 16), (0, 1, 3, 5, 7, 11, 14, 17)),
 'split': ((0, 0, 0, 0, 0, 2, 0, 0, 0, 0, 0, 0, 0, 0, 2, 0, 2, 0, 0, 0),
           (0, 0, 0, 0, 0, 0, 0, 0, 0, 0, 0, 2, 0, 0, 1, 0, 0, 0, 0, 0, 0, 0, 0, 0, 0, 0, 0)),
 'src': ((11, 0, 0, 0, 1, 1, 0, 2, 3, 1, 0, 1, 13, 13, 6, 0, 13, 0, 1, 0, 1, 1, 0, 2, 3, 1, 0, 1, 11, 11, 6, 0),
         (0, 0, 10, 10, 12, 12, 10, 1, 0, 10, 10, 1, 12, 12, 12, 10, 0, 10, 12, 10, 12, 12, 12, 10, 7, 7, 7, 10, 0, 0,
          12, 10),
         (13, 11, 0, 13, 0, 0, 0, 11, 11, 11, 6, 11, 13, 13, 0, 13, 11, 13, 0, 11, 0, 0, 0, 13, 13, 13, 6, 13, 11, 11,
          0, 11),
         (0, 10, 12, 10, 12, 12, 12, 10, 7, 7, 7, 10, 0, 0, 12, 10, 0, 0, 10, 10, 12, 12, 10, 1, 0, 10, 10, 1, 12, 12,
          12, 10)),
 'tail': (((('m', 3, 31), ('m', 1, 15), ('m', 3, 3), ('m', 1, 19), ('f', 19), ('f', 3), ('f', 7), ('f', 23), ('f', 33),
            ('f', 32), ('f', 31), ('f', 15), ('m', 1, 6), ('m', 3, 22), ('f', 6), ('f', 22), ('m', 1, 30), ('m', 3, 14),
            ('m', 3, 11), ('m', 1, 23), ('m', 3, 33), ('m', 1, 32), ('m', 3, 15), ('m', 1, 31), ('f', 30), ('f', 14),
            ('f', 2), ('f', 18), ('m', 1, 17), ('m', 3, 1), ('f', 17), ('f', 1), ('f', 10), ('f', 26), ('m', 1, 29),
            ('m', 3, 13), ('f', 29), ('f', 13), ('m', 1, 11), ('m', 3, 27), ('m', 3, 32), ('m', 1, 33), ('m', 3, 19),
            ('m', 1, 3), ('m', 3, 17), ('m', 1, 1), ('m', 3, 23), ('m', 1, 7), ('f', 11), ('f', 27), ('f', 9),
            ('f', 25), ('f', 5), ('f', 21), ('f', 28), ('f', 12), ('m', 1, 8), ('m', 3, 24), ('f', 8), ('f', 24),
            ('f', 16), ('f', 0), ('ws', 'early'), ('f', 4), ('f', 20), ('ws', 'late')),
           ((3, 24), (1, 8))),
          ((('m', 2, 21), ('m', 2, 15), ('m', 2, 0), ('m', 2, 12), ('m', 2, 27), ('f', 18), ('f', 14), ('f', 26),
            ('m', 0, 21), ('f', 22), ('f', 13), ('f', 27), ('f', 15), ('f', 25), ('f', 19), ('f', 21), ('f', 6),
            ('m', 0, 12), ('f', 12), ('f', 30), ('m', 0, 24), ('f', 24), ('m', 2, 32), ('m', 2, 23), ('m', 2, 24),
            ('f', 23), ('m', 0, 0), ('m', 2, 13), ('f', 32), ('f', 0), ('f', 31), ('m', 0, 20), ('f', 20), ('f', 17),
            ('f', 10), ('f', 29), ('f', 2), ('f', 11), ('f', 33), ('f', 4), ('m', 2, 3), ('f', 3), ('f', 9),
            ('m', 2, 1), ('f', 1), ('f', 5), ('f', 7), ('f', 16), ('ws', 'early'), ('f', 8), ('f', 28),
            ('ws', 'late')),
           ()),
          ((('m', 3, 8), ('m', 1, 24), ('m', 3, 16), ('m', 1, 0), ('f', 2), ('f', 18), ('m', 1, 20), ('m', 3, 4),
            ('f', 30), ('f', 14), ('m', 1, 10), ('m', 3, 26), ('m', 3, 18), ('m', 1, 2), ('f', 10), ('f', 26), ('f', 6),
            ('f', 22), ('m', 1, 4), ('m', 3, 20), ('f', 4), ('f', 20), ('m', 1, 9), ('m', 3, 25), ('f', 9), ('f', 25),
            ('m', 1, 5), ('m', 3, 21), ('f', 5), ('f', 21), ('f', 31), ('f', 15), ('m', 1, 16), ('m', 3, 0), ('f', 16),
            ('f', 0), ('m', 1, 28), ('m', 3, 12), ('f', 28), ('f', 12), ('f', 11), ('f', 27), ('f', 33), ('f', 32),
            ('f', 7), ('f', 23), ('f', 8), ('f', 24), ('f', 29), ('f', 13), ('f', 19), ('f', 3), ('ws', 'early'),
            ('f', 17), ('f', 1), ('ws', 'late')),
           ()),
          ((('m', 2, 5), ('m', 2, 31), ('m', 2, 16), ('m', 2, 28), ('f', 2), ('f', 30), ('f', 10), ('f', 6),
            ('m', 0, 5), ('f', 29), ('f', 7), ('f', 31), ('f', 9), ('f', 3), ('f', 5), ('f', 22), ('m', 0, 28),
            ('f', 28), ('f', 14), ('m', 0, 8), ('m', 2, 11), ('f', 8), ('m', 2, 33), ('m', 2, 7), ('m', 2, 8),
            ('m', 2, 29), ('f', 11), ('m', 0, 16), ('f', 33), ('f', 16), ('f', 15), ('m', 0, 4), ('f', 4), ('f', 1),
            ('f', 26), ('f', 13), ('f', 18), ('f', 27), ('f', 32), ('f', 20), ('m', 2, 19), ('f', 19), ('f', 25),
            ('m', 2, 17), ('ws', 'early'), ('f', 17), ('f', 21), ('f', 23), ('f', 0), ('f', 24), ('f', 12),
            ('ws', 'late')),
           ((2, 19), (2, 17)))),
 'tiles': ((0, 0, 0, 64, 'A1'), (0, 1, 0, 64, 'B0'), (0, 2, 0, 64, 'B1'), (0, 3, 0, 64, 'B0'), (1, 0, 0, 64, 'B1'),
           (1, 1, 0, 64, 'B1'), (1, 2, 0, 64, 'A0'), (1, 3, 0, 64, 'A0'), (2, 0, 0, 64, 'P1'), (2, 1, 0, 64, 'B1'),
           (2, 2, 0, 64, 'B1'), (2, 3, 0, 64, 'P1'), (3, 0, 0, 64, 'A1'), (3, 1, 0, 64, 'P3'), (3, 2, 0, 64, 'B0'),
           (3, 3, 0, 32, 'B0'), (4, 0, 0, 64, 'B1'), (4, 1, 0, 64, 'A0'), (4, 2, 0, 64, 'A1'), (4, 3, 0, 64, 'A0'),
           (5, 0, 0, 64, 'A1'), (5, 1, 0, 64, 'A1'), (5, 2, 0, 64, 'B0'), (5, 3, 0, 64, 'B0'), (6, 0, 0, 64, 'P3'),
           (6, 1, 0, 64, 'A1'), (6, 2, 0, 64, 'A1'), (6, 3, 0, 64, 'P3'), (7, 0, 0, 64, 'B1'), (7, 1, 0, 64, 'P1'),
           (7, 2, 0, 64, 'A0'), (7, 3, 0, 32, 'A0'), (3, 3, 32, 32, 'P3'), (7, 3, 32, 32, 'P1')),
 'w1o': ((2, 1, 3, 0), (0, 3, 1, 2), (2, 1, 0, 3), (0, 3, 1, 2)),
 'w2o': ((2, 0, 1, 3), (3, 2, 1, 0), (3, 2, 1, 0), (3, 2, 1, 0)),
 'xm': (((3, 3, 3), (1, 7, 3), (3, 0, 3), (1, 4, 3), (3, 4, 3), (1, 0, 3), (3, 0, 1), (1, 4, 1), (3, 6, 1), (3, 5, 2),
         (3, 6, 2), (3, 4, 2), (3, 7, 3), (1, 2, 1), (1, 1, 2), (1, 2, 2), (1, 0, 2), (1, 3, 3), (1, 5, 3), (1, 6, 3),
         (3, 1, 3), (3, 2, 3)),
        ((2, 7, 1), (0, 0, 0), (2, 0, 1), (0, 7, 0), (2, 4, 0), (0, 7, 1), (2, 7, 0), (2, 4, 3), (2, 1, 3), (2, 7, 3),
         (2, 2, 3), (2, 2, 0), (2, 2, 1)),
        ((3, 1, 0), (1, 5, 0), (3, 5, 1), (1, 1, 1), (3, 5, 0), (1, 1, 0), (1, 4, 2), (1, 7, 2), (1, 5, 1), (1, 5, 2),
         (3, 0, 2), (3, 3, 2), (3, 1, 1), (3, 1, 2), (1, 3, 0), (3, 7, 0), (1, 3, 2), (3, 7, 2), (1, 3, 1), (3, 7, 1)),
        ((2, 3, 1), (0, 4, 0), (2, 4, 1), (0, 3, 0), (2, 0, 0), (0, 3, 1), (2, 3, 0), (2, 0, 3), (2, 5, 3), (2, 3, 3),
         (2, 6, 3), (2, 6, 0), (2, 6, 1))),
 'xord': ((6, 5, 1, 3, 7, 0, 4, 2), (5, 3, 4, 2, 1, 7, 0, 6), (1, 5, 7, 2, 3, 4, 0, 6), (1, 7, 0, 6, 5, 3, 4, 2))}


def pallas_dist_mlp2_tp_i_m512_h1024_out512_kernel(x, W1, W2):
    return build(PLAN)(x, W1, W2)
```
